```python
import numpy as np

kernel_name = "dist_moe_shared_ep_outshard_n512_d256_e2_h512"

def setup_inputs():
    x = np.random.randn(512, 256).astype(np.float32)
    router_W = np.random.randn(256, 8).astype(np.float32) * 0.1
    scores64 = x.astype(np.float64) @ router_W.astype(np.float64)
    route_idx = np.argsort(-scores64, axis=-1)[:, :1].astype(np.int32)
    expert_W = np.random.randn(8, 256, 512).astype(np.float32) * 0.02
    shared_W = np.random.randn(256, 512).astype(np.float32) * 0.02
    return {"x": x, "router_W": router_W, "route_idx": route_idx, "expert_W": expert_W, "shared_W": shared_W}

def reference(x, router_W, route_idx, expert_W, shared_W):
    scores = x @ router_W
    s_max = scores.max(axis=-1, keepdims=True)
    probs = np.exp(scores - s_max)
    probs = probs / probs.sum(axis=-1, keepdims=True)
    shared = x @ shared_W
    out = np.zeros((512, 512), dtype=np.float32)
    for i in range(512):
        e = int(route_idx[i, 0])
        out[i] = shared[i] + probs[i, e] * (x[i] @ expert_W[e])
    return out
```

```python
import jax
import jax.numpy as jnp
from jax import lax
from jax.experimental import pallas as pl
from jax.experimental.pallas import tpu as pltpu

N_DEV = 4
N_TOK = 512
D = 256
H = 512
N_EXP = 8
E_LOC = N_EXP // N_DEV
ROWS = N_TOK // N_DEV


def pallas_dist_moe_shared_ep_outshard_n512_d256_e2_h512_kernel(
    x: jax.Array,
    router_W: jax.Array,
    route_idx: jax.Array,
    expert_W: jax.Array,
    shared_W: jax.Array,
):
    def body(x_hbm, ew_hbm, sw_hbm, rw_ref, ridx_ref, out_ref,
             x_v, ew_v, sw_v, gate_v, send_buf, recv_buf,
             load_sems, send_sems, recv_sems):
        my = lax.axis_index("i")

        cp_x = pltpu.make_async_copy(x_hbm, x_v, load_sems.at[0])
        cp_ew = pltpu.make_async_copy(ew_hbm, ew_v, load_sems.at[1])
        cp_sw = pltpu.make_async_copy(sw_hbm, sw_v, load_sems.at[2])
        cp_x.start()
        cp_ew.start()
        cp_sw.start()

        cp_x.wait()
        xf = x_v[...]
        scores = jnp.dot(xf, rw_ref[...], preferred_element_type=jnp.float32,
                         precision=lax.Precision.HIGHEST)
        s_max = jnp.max(scores, axis=-1, keepdims=True)
        p = jnp.exp(scores - s_max)
        probs = p / jnp.sum(p, axis=-1, keepdims=True)
        ridx = ridx_ref[...]
        col = lax.broadcasted_iota(jnp.int32, (N_TOK, N_EXP), 1)
        for j in range(E_LOC):
            e = my * E_LOC + j
            sel = jnp.logical_and(col == e, ridx == e)
            gate_v[j] = jnp.sum(jnp.where(sel, probs, 0.0), axis=-1,
                                keepdims=True)

        cp_ew.wait()
        w0 = ew_v[0].astype(jnp.bfloat16)
        w1 = ew_v[1].astype(jnp.bfloat16)

        def partial_block(blk):
            start = pl.multiple_of(blk * ROWS, ROWS)
            xb = x_v[pl.ds(start, ROWS), :].astype(jnp.bfloat16)
            g0 = gate_v[0, pl.ds(start, ROWS), :]
            g1 = gate_v[1, pl.ds(start, ROWS), :]
            y0 = jnp.dot(xb, w0, preferred_element_type=jnp.float32)
            y1 = jnp.dot(xb, w1, preferred_element_type=jnp.float32)
            return g0 * y0 + g1 * y1

        rdmas = []
        for k in range(1, N_DEV):
            dst = lax.rem(my + k, N_DEV)
            send_buf[k - 1] = partial_block(dst).astype(jnp.bfloat16)
            rdma = pltpu.make_async_remote_copy(
                src_ref=send_buf.at[k - 1],
                dst_ref=recv_buf.at[k - 1],
                send_sem=send_sems.at[k - 1],
                recv_sem=recv_sems.at[k - 1],
                device_id=(dst,),
                device_id_type=pl.DeviceIdType.MESH,
            )
            rdma.start()
            rdmas.append(rdma)

        acc = partial_block(my)
        cp_sw.wait()
        start = pl.multiple_of(my * ROWS, ROWS)
        xb = x_v[pl.ds(start, ROWS), :].astype(jnp.bfloat16)
        acc = acc + jnp.dot(xb, sw_v[...].astype(jnp.bfloat16),
                            preferred_element_type=jnp.float32)

        for k in range(1, N_DEV):
            rdmas[k - 1].wait_recv()
            acc = acc + recv_buf[k - 1].astype(jnp.float32)
        out_ref[...] = acc

        for k in range(1, N_DEV):
            rdmas[k - 1].wait_send()

    return pl.pallas_call(
        body,
        out_shape=jax.ShapeDtypeStruct((ROWS, H), jnp.float32),
        in_specs=[
            pl.BlockSpec(memory_space=pl.ANY),
            pl.BlockSpec(memory_space=pl.ANY),
            pl.BlockSpec(memory_space=pl.ANY),
            pl.BlockSpec(memory_space=pltpu.VMEM),
            pl.BlockSpec(memory_space=pltpu.VMEM),
        ],
        out_specs=pl.BlockSpec(memory_space=pltpu.VMEM),
        scratch_shapes=[
            pltpu.VMEM((N_TOK, D), jnp.float32),
            pltpu.VMEM((E_LOC, D, H), jnp.float32),
            pltpu.VMEM((D, H), jnp.float32),
            pltpu.VMEM((E_LOC, N_TOK, 1), jnp.float32),
            pltpu.VMEM((N_DEV - 1, ROWS, H), jnp.bfloat16),
            pltpu.VMEM((N_DEV - 1, ROWS, H), jnp.bfloat16),
            pltpu.SemaphoreType.DMA((3,)),
            pltpu.SemaphoreType.DMA((N_DEV - 1,)),
            pltpu.SemaphoreType.DMA((N_DEV - 1,)),
        ],
    )(x, expert_W, shared_W, router_W, route_idx)
```

```python
import jax
import jax.numpy as jnp
from jax import lax
from jax.experimental import pallas as pl
from jax.experimental.pallas import tpu as pltpu

N_DEV = 4
N_TOK = 512
D = 256
H = 512
N_EXP = 8
E_LOC = N_EXP // N_DEV
ROWS = N_TOK // N_DEV
N_REM = N_DEV - 1

NQ = 4
QW = H // NQ
CH = 16
NCH = ROWS // CH
SLOT_ORDER = (1, 0, 2)
SCOPES = False


class _Null:
    def __enter__(self):
        return self

    def __exit__(self, *a):
        return False


def _scope(name):
    return jax.named_scope(name) if SCOPES else _Null()


def pallas_dist_moe_shared_ep_outshard_n512_d256_e2_h512_kernel(
    x: jax.Array,
    router_W: jax.Array,
    route_idx: jax.Array,
    expert_W: jax.Array,
    shared_W: jax.Array,
):
    f32, bf16, i32 = jnp.float32, jnp.bfloat16, jnp.int32

    def body(x_hbm, ew_hbm, sw_hbm, rwt_hbm, ridx_hbm, out_ref,
             ridx_v, rwt_v, xs_v, xg_v, ew_v, sw_v, send_buf, recv_buf,
             ld_sems, send_sems, recv_sems):
        my = lax.axis_index("i")

        cp_ridx = pltpu.make_async_copy(ridx_hbm, ridx_v, ld_sems.at[0])
        cp_rwt = pltpu.make_async_copy(rwt_hbm, rwt_v, ld_sems.at[1])
        cp_ridx.start()
        cp_rwt.start()
        cp_x = []
        for s in range(N_DEV):
            blk = lax.rem(my + 1 + s, N_DEV)
            start = pl.multiple_of(blk * ROWS, ROWS)
            cp_x.append(pltpu.make_async_copy(
                x_hbm.at[pl.ds(start, ROWS)],
                xs_v.at[pl.ds(s * ROWS, ROWS)], ld_sems.at[2 + s]))
        cp_w = [pltpu.make_async_copy(ew_hbm.at[:, :, pl.ds(q * QW, QW)],
                                      ew_v.at[q], ld_sems.at[6 + q])
                for q in range(NQ)]
        cp_sw = pltpu.make_async_copy(sw_hbm, sw_v, ld_sems.at[6 + NQ])
        for s in range(N_REM):
            cp_x[s].start()
        for q in range(NQ):
            cp_w[q].start()
        cp_x[N_REM].start()
        cp_sw.start()

        recv_buf[...] = jnp.zeros(recv_buf.shape, bf16)
        bsem = pltpu.get_barrier_semaphore()
        for k in range(1, N_DEV):
            pl.semaphore_signal(bsem, inc=1,
                                device_id=(lax.rem(my + k, N_DEV),),
                                device_id_type=pl.DeviceIdType.MESH)

        with _scope("W_ridx"):
            cp_ridx.wait()
        r4 = ridx_v[...]
        sub4 = lax.broadcasted_iota(i32, (N_DEV, ROWS), 0)
        rows = [jnp.sum(jnp.where(sub4 == lax.rem(my + 1 + s, N_DEV), r4, 0),
                        axis=0, keepdims=True) for s in range(N_DEV)]
        rs8 = jnp.concatenate(rows + [jnp.full((4, ROWS), -1, i32)], axis=0)
        owner8 = lax.shift_right_arithmetic(rs8, 1)
        tri = (lax.broadcasted_iota(i32, (ROWS, ROWS), 0)
               < lax.broadcasted_iota(i32, (ROWS, ROWS), 1)).astype(bf16)
        rank8 = jnp.zeros((8, ROWS), f32)
        for o in range(N_DEV):
            mo = owner8 == o
            pre = jnp.dot(mo.astype(bf16), tri, preferred_element_type=f32)
            rank8 = rank8 + jnp.where(mo, pre, 0.0)
        rank8 = rank8.astype(i32)

        mine8 = owner8 == my
        key8 = jnp.where(mine8, rank8, -1)
        sub_r = lax.broadcasted_iota(i32, (ROWS, ROWS), 0)
        n_send, n_recv = [], []
        for s in range(N_REM):
            cnt = jnp.sum(mine8[s:s + 1, :].astype(i32))
            n_send.append((cnt + (CH - 1)) // CH)
        own_row = owner8[N_REM:N_REM + 1, :]
        slot_of = (my + (N_DEV - 1) - own_row) & (N_DEV - 1)
        for s in range(N_REM):
            cnt = jnp.sum(
                (jnp.logical_and(slot_of == s, own_row != my)).astype(i32))
            n_recv.append((cnt + (CH - 1)) // CH)
        pos_row = jnp.where(own_row == my, -1,
                            slot_of * ROWS + rank8[N_REM:N_REM + 1, :])

        with _scope("W_rwt"):
            cp_rwt.wait()
        rw = rwt_v[...]
        rw_hi = rw.astype(bf16)
        rw_lo = (rw - rw_hi.astype(f32)).astype(bf16)
        rw_cat = jnp.concatenate([rw_hi, rw_lo], axis=0)
        nt = (((1,), (1,)), ((), ()))

        def gate_rows(xf, ridx_row):
            n = xf.shape[0]
            x_hi = xf.astype(bf16)
            x_lo = (xf - x_hi.astype(f32)).astype(bf16)
            a = lax.dot_general(rw_cat, x_hi, nt, preferred_element_type=f32)
            b = lax.dot_general(rw_hi, x_lo, nt, preferred_element_type=f32)
            sc = a[0:N_EXP] + a[N_EXP:2 * N_EXP] + b
            mx = jnp.max(sc, axis=0, keepdims=True)
            ex = jnp.exp(sc - mx)
            pr = ex / jnp.sum(ex, axis=0, keepdims=True)
            sub = lax.broadcasted_iota(i32, (N_EXP, n), 0)
            out = []
            for e in range(E_LOC):
                eg = my * E_LOC + e
                sel = jnp.logical_and(sub == eg, ridx_row == eg)
                out.append(jnp.sum(jnp.where(sel, pr, 0.0), axis=0,
                                   keepdims=True))
            return out

        with _scope("W_x"):
            for s in range(N_REM):
                cp_x[s].wait()
        xr = xs_v[0:N_REM * ROWS, :]
        ridx_rem = jnp.concatenate([rs8[s:s + 1, :] for s in range(N_REM)],
                                   axis=1)
        g0, g1 = gate_rows(xr, ridx_rem)
        stack = []
        for s in range(N_REM):
            stack += [g0[:, s * ROWS:(s + 1) * ROWS],
                      g1[:, s * ROWS:(s + 1) * ROWS]]
        stack += [pos_row.astype(f32), jnp.zeros((1, ROWS), f32)]
        gcol = jnp.concatenate(stack, axis=0).T

        for s in range(N_REM):
            xs = xr[s * ROWS:(s + 1) * ROWS, :]
            xg = jnp.concatenate([gcol[:, 2 * s:2 * s + 1] * xs,
                                  gcol[:, 2 * s + 1:2 * s + 2] * xs],
                                 axis=1).astype(bf16)
            p = (key8[s:s + 1, :] == sub_r).astype(bf16)
            xg_v[s * ROWS:(s + 1) * ROWS, :] = jnp.dot(
                p, xg, preferred_element_type=f32).astype(bf16)

        def rdma(s, q, n):
            rows_ = pl.ds(s * ROWS, n * CH)
            idx = q * N_REM + s
            return pltpu.make_async_remote_copy(
                src_ref=send_buf.at[q, rows_, :],
                dst_ref=recv_buf.at[q, rows_, :],
                send_sem=send_sems.at[idx],
                recv_sem=recv_sems.at[idx],
                device_id=(lax.rem(my + 1 + s, N_DEV),),
                device_id_type=pl.DeviceIdType.MESH)

        def by_size(n_dyn, fn):
            branches = [lambda: None] + [
                (lambda n=n: fn(n)) for n in range(1, NCH + 1)]
            lax.switch(n_dyn, branches)

        for q in range(NQ):
            with _scope(f"W_w{q}"):
                cp_w[q].wait()
            wq = ew_v[q].reshape(E_LOC * D, QW).astype(bf16)
            send_buf[q] = jnp.dot(xg_v[...], wq,
                                  preferred_element_type=f32).astype(bf16)
            if q == 0:
                with _scope("W_barrier"):
                    pl.semaphore_wait(bsem, N_REM)
            with _scope(f"issue{q}"):
                for s in SLOT_ORDER:
                    by_size(n_send[s],
                            lambda n, s=s, q=q: rdma(s, q, n).start())

        with _scope("W_xo"):
            cp_x[N_REM].wait()
        xo = xs_v[N_REM * ROWS:N_DEV * ROWS, :]
        go0, go1 = gate_rows(xo, rs8[N_REM:N_REM + 1, :])
        gocol = jnp.concatenate(
            [go0, go1, jnp.zeros((6, ROWS), f32)], axis=0).T
        xo_cat = jnp.concatenate([gocol[:, 0:1] * xo, gocol[:, 1:2] * xo, xo],
                                 axis=1).astype(bf16)
        lane = lax.broadcasted_iota(i32, (ROWS, N_REM * ROWS), 1)
        qcat = (gcol[:, 6:7].astype(i32) == lane).astype(bf16)
        with _scope("W_sw"):
            cp_sw.wait()
        for q in range(NQ):
            wcat = jnp.concatenate(
                [ew_v[q].reshape(E_LOC * D, QW),
                 sw_v[:, q * QW:(q + 1) * QW]], axis=0).astype(bf16)
            out_ref[:, q * QW:(q + 1) * QW] = jnp.dot(
                xo_cat, wcat, preferred_element_type=f32)

        for q in range(NQ):
            with _scope(f"W_recv{q}"):
                for s in range(N_REM):
                    by_size(n_recv[s],
                            lambda n, s=s, q=q: rdma(s, q, n).wait_recv())
            out_ref[:, q * QW:(q + 1) * QW] += jnp.dot(
                qcat, recv_buf[q], preferred_element_type=f32)

        with _scope("W_send"):
            for q in range(NQ):
                for s in range(N_REM):
                    by_size(n_send[s],
                            lambda n, s=s, q=q: rdma(s, q, n).wait_send())

    n_remote = NQ * N_REM
    return pl.pallas_call(
        body,
        out_shape=jax.ShapeDtypeStruct((ROWS, H), f32),
        in_specs=[pl.BlockSpec(memory_space=pltpu.HBM)] * 5,
        out_specs=pl.BlockSpec(memory_space=pltpu.VMEM),
        scratch_shapes=[
            pltpu.VMEM((N_DEV, ROWS), i32),
            pltpu.VMEM((N_EXP, D), f32),
            pltpu.VMEM((N_TOK, D), f32),
            pltpu.VMEM((N_REM * ROWS, E_LOC * D), bf16),
            pltpu.VMEM((NQ, E_LOC, D, QW), f32),
            pltpu.VMEM((D, H), f32),
            pltpu.VMEM((NQ, N_REM * ROWS, QW), bf16),
            pltpu.VMEM((NQ, N_REM * ROWS, QW), bf16),
            pltpu.SemaphoreType.DMA((7 + NQ,)),
            pltpu.SemaphoreType.DMA((n_remote,)),
            pltpu.SemaphoreType.DMA((n_remote,)),
        ],
        compiler_params=pltpu.CompilerParams(collective_id=0),
    )(x, expert_W, shared_W, router_W.T,
      route_idx.astype(jnp.int32).reshape(N_DEV, ROWS))
```

```python
import jax
import jax.numpy as jnp
from jax import lax
from jax.experimental import pallas as pl
from jax.experimental.pallas import tpu as pltpu

N_DEV = 4
N_TOK = 512
D = 256
H = 512
N_EXP = 8
E_LOC = N_EXP // N_DEV
ROWS = N_TOK // N_DEV
N_REM = N_DEV - 1

NQ = 4
QW = H // NQ
CH = 16
NCH = ROWS // CH
CAP_FAST = 48
DEFER = NQ
SCOPES = False


class _Null:
    def __enter__(self):
        return self

    def __exit__(self, *a):
        return False


def _scope(name):
    return jax.named_scope(name) if SCOPES else _Null()


def pallas_dist_moe_shared_ep_outshard_n512_d256_e2_h512_kernel(
    x: jax.Array,
    router_W: jax.Array,
    route_idx: jax.Array,
    expert_W: jax.Array,
    shared_W: jax.Array,
):
    f32, bf16, i32 = jnp.float32, jnp.bfloat16, jnp.int32

    def body(x_hbm, ew_hbm, sw_hbm, rwt_hbm, ridx_hbm, out_ref,
             ridx_v, rwt_v, xs_v, ew_v, sw_v, send_buf, recv_buf,
             ld_sems, send_sems, recv_sems):
        my = lax.axis_index("i")
        odd = my & 1
        peer = [lax.rem(my + 2, N_DEV),
                lax.rem(my + 1 + 2 * odd, N_DEV),
                lax.rem(my + 3 - 2 * odd, N_DEV),
                my]

        cp_ridx = pltpu.make_async_copy(ridx_hbm, ridx_v, ld_sems.at[0])
        cp_rwt = pltpu.make_async_copy(rwt_hbm, rwt_v, ld_sems.at[1])
        cp_ridx.start()
        cp_rwt.start()
        cp_x = []
        for s in range(N_DEV):
            start = pl.multiple_of(peer[s] * ROWS, ROWS)
            cp_x.append(pltpu.make_async_copy(
                x_hbm.at[pl.ds(start, ROWS)],
                xs_v.at[pl.ds(s * ROWS, ROWS)], ld_sems.at[2 + s]))
        cp_w = [pltpu.make_async_copy(ew_hbm.at[:, :, pl.ds(q * QW, QW)],
                                      ew_v.at[q], ld_sems.at[6 + q])
                for q in range(NQ)]
        cp_sw = pltpu.make_async_copy(sw_hbm, sw_v, ld_sems.at[6 + NQ])
        for s in range(N_REM):
            cp_x[s].start()
        for q in range(NQ):
            cp_w[q].start()
        cp_x[N_REM].start()
        cp_sw.start()

        recv_buf[...] = jnp.zeros(recv_buf.shape, bf16)
        bsem = pltpu.get_barrier_semaphore()
        for k in range(1, N_DEV):
            pl.semaphore_signal(bsem, inc=1,
                                device_id=(lax.rem(my + k, N_DEV),),
                                device_id_type=pl.DeviceIdType.MESH)

        with _scope("W_ridx"):
            cp_ridx.wait()
        r4 = ridx_v[...]
        sub4 = lax.broadcasted_iota(i32, (N_DEV, ROWS), 0)
        rows = [jnp.sum(jnp.where(sub4 == peer[s], r4, 0),
                        axis=0, keepdims=True) for s in range(N_DEV)]
        rs8 = jnp.concatenate(rows + [jnp.full((4, ROWS), -1, i32)], axis=0)
        owner8 = lax.shift_right_arithmetic(rs8, 1)
        tri = (lax.broadcasted_iota(i32, (ROWS, ROWS), 0)
               < lax.broadcasted_iota(i32, (ROWS, ROWS), 1)).astype(bf16)
        rank8 = jnp.zeros((8, ROWS), f32)
        for o in range(N_DEV):
            mo = owner8 == o
            pre = jnp.dot(mo.astype(bf16), tri, preferred_element_type=f32)
            rank8 = rank8 + jnp.where(mo, pre, 0.0)
        rank8 = rank8.astype(i32)

        mine8 = owner8 == my
        key8 = jnp.where(mine8, rank8, -1)
        n_send, n_recv = [], []
        for s in range(N_DEV):
            cnt = jnp.sum(mine8[s:s + 1, :].astype(i32))
            n_send.append((cnt + (CH - 1)) // CH)
        own_row = owner8[N_REM:N_REM + 1, :]
        slot_of = jnp.full_like(own_row, N_REM)
        for s in range(N_REM):
            slot_of = jnp.where(own_row == peer[s], s, slot_of)
        for s in range(N_REM):
            cnt = jnp.sum((slot_of == s).astype(i32))
            n_recv.append((cnt + (CH - 1)) // CH)
        pos_row = slot_of * ROWS + rank8[N_REM:N_REM + 1, :]

        with _scope("W_rwt"):
            cp_rwt.wait()
        rw = rwt_v[...]
        rw_hi = rw.astype(bf16)
        rw_lo = (rw - rw_hi.astype(f32)).astype(bf16)
        rw_cat = jnp.concatenate(
            [jnp.concatenate([rw_hi, rw_hi], axis=1),
             jnp.concatenate([rw_lo, jnp.zeros_like(rw_lo)], axis=1)],
            axis=0)
        nt = (((1,), (1,)), ((), ()))

        def split(xf):
            hi = xf.astype(bf16)
            lo = (xf - hi.astype(f32)).astype(bf16)
            return jnp.concatenate([hi, lo], axis=1)

        def probs_t(x_hl):
            a = lax.dot_general(rw_cat, x_hl, nt, preferred_element_type=f32)
            sc = a[0:N_EXP] + a[N_EXP:2 * N_EXP]
            mx = jnp.max(sc, axis=0, keepdims=True)
            ex = jnp.exp(sc - mx)
            return ex / jnp.sum(ex, axis=0, keepdims=True)

        def local_gates(gsel):
            sub = lax.broadcasted_iota(i32, gsel.shape, 0)
            return [jnp.sum(jnp.where(sub == my * E_LOC + e, gsel, 0.0),
                            axis=0, keepdims=True) for e in range(E_LOC)]

        def rdma(s, q, n, stride):
            idx = q * N_REM + s
            return pltpu.make_async_remote_copy(
                src_ref=send_buf.at[q, pl.ds(s * stride, n * CH), :],
                dst_ref=recv_buf.at[q, pl.ds(s * ROWS, n * CH), :],
                send_sem=send_sems.at[idx],
                recv_sem=recv_sems.at[idx],
                device_id=(peer[s],),
                device_id_type=pl.DeviceIdType.MESH)

        def by_size(n_dyn, n_max, fn, lo=0):
            if lo == n_max:
                if lo > 0:
                    fn(lo)
                return
            mid = (lo + n_max) // 2
            lax.cond(n_dyn <= mid,
                     lambda: by_size(n_dyn, mid, fn, lo),
                     lambda: by_size(n_dyn, n_max, fn, mid + 1))

        def send_phase(cap):
            m = N_REM * cap
            sub_c = lax.broadcasted_iota(i32, (cap, ROWS), 0)
            sub_e = lax.broadcasted_iota(i32, (N_EXP, ROWS), 0)
            ps = [(key8[s:s + 1, :] == sub_c).astype(bf16)
                  for s in range(N_DEV)]
            sels = [lax.dot_general(
                (sub_e == rs8[s:s + 1, :]).astype(bf16), ps[s], nt,
                preferred_element_type=f32) for s in range(N_DEV)]

            def compact(slots):
                xcs = [jnp.dot(ps[s], split(xs_v[s * ROWS:(s + 1) * ROWS, :]),
                               preferred_element_type=f32).astype(bf16)
                       for s in slots]
                xh = jnp.concatenate([xc[:, 0:D] for xc in xcs], axis=0)
                gts = []
                for s, xc in zip(slots, xcs):
                    g0, g1 = local_gates(probs_t(xc) * sels[s])
                    gts.append(jnp.concatenate(
                        [g0, g1, jnp.zeros((8 - E_LOC, cap), f32)], axis=0).T)
                gc0 = jnp.concatenate([g[:, 0:1] for g in gts], axis=0)
                gc1 = jnp.concatenate([g[:, 1:2] for g in gts], axis=0)
                return xh, gc0, gc1

            def experts(q, xh, gc0, gc1):
                wq = jnp.concatenate([ew_v[q, 0], ew_v[q, 1]],
                                     axis=1).astype(bf16)
                yy = jnp.dot(xh, wq, preferred_element_type=f32)
                return (gc0 * yy[:, 0:QW]
                        + gc1 * yy[:, QW:2 * QW]).astype(bf16)

            with _scope("W_x"):
                for s in range(N_REM):
                    cp_x[s].wait()
            rem = compact(range(N_REM))
            for q in range(NQ):
                with _scope(f"W_w{q}"):
                    cp_w[q].wait()
                send_buf[q, 0:m, :] = experts(q, *rem)
                if q == 0:
                    with _scope("W_barrier"):
                        pl.semaphore_wait(bsem, N_REM)
                with _scope(f"issue{q}"):
                    for s, qq in ((0, q), (1, q), (2, q - DEFER)):
                        if qq >= 0:
                            by_size(n_send[s], cap // CH,
                                    lambda n, s=s, qq=qq:
                                    rdma(s, qq, n, cap).start())
            for qq in range(max(NQ - DEFER, 0), NQ):
                by_size(n_send[2], cap // CH,
                        lambda n, qq=qq: rdma(2, qq, n, cap).start())

            with _scope("W_xo"):
                cp_x[N_REM].wait()
            own = compact([N_REM])
            for q in range(NQ):
                recv_buf[q, N_REM * ROWS:N_REM * ROWS + cap, :] = experts(q, *own)

        n_max = jnp.maximum(jnp.maximum(n_send[0], n_send[1]),
                            jnp.maximum(n_send[2], n_send[3]))
        lax.cond(n_max <= CAP_FAST // CH,
                 lambda: send_phase(CAP_FAST),
                 lambda: send_phase(ROWS))

        posc = jnp.concatenate(
            [pos_row.astype(f32), jnp.zeros((7, ROWS), f32)], axis=0).T
        lane = lax.broadcasted_iota(i32, (ROWS, N_DEV * ROWS), 1)
        qcat = (posc[:, 0:1].astype(i32) == lane).astype(bf16)
        with _scope("W_sw"):
            cp_sw.wait()
        out_ref[...] = jnp.dot(
            xs_v[N_REM * ROWS:N_DEV * ROWS, :].astype(bf16),
            sw_v[...].astype(bf16), preferred_element_type=f32)

        with _scope("W_send"):
            for s in range(N_REM):
                def waits(n, s=s):
                    for q in range(NQ):
                        rdma(s, q, n, ROWS).wait_send()
                by_size(n_send[s], NCH, waits)

        def scatter_add(q):
            out_ref[:, q * QW:(q + 1) * QW] += jnp.dot(
                qcat, recv_buf[q], preferred_element_type=f32)

        with _scope("W_recvA"):
            for s in range(N_REM):
                def waits(n, s=s):
                    for q in range(NQ - 1):
                        rdma(s, q, n, ROWS).wait_recv()
                by_size(n_recv[s], NCH, waits)
        for q in range(NQ - 1):
            scatter_add(q)
        with _scope("W_recvB"):
            for s in range(N_REM):
                by_size(n_recv[s], NCH,
                        lambda n, s=s: rdma(s, NQ - 1, n, ROWS).wait_recv())
        scatter_add(NQ - 1)

    n_remote = NQ * N_REM
    return pl.pallas_call(
        body,
        out_shape=jax.ShapeDtypeStruct((ROWS, H), f32),
        in_specs=[pl.BlockSpec(memory_space=pltpu.HBM)] * 5,
        out_specs=pl.BlockSpec(memory_space=pltpu.VMEM),
        scratch_shapes=[
            pltpu.VMEM((N_DEV, ROWS), i32),
            pltpu.VMEM((N_EXP, D), f32),
            pltpu.VMEM((N_TOK, D), f32),
            pltpu.VMEM((NQ, E_LOC, D, QW), f32),
            pltpu.VMEM((D, H), f32),
            pltpu.VMEM((NQ, N_REM * ROWS, QW), bf16),
            pltpu.VMEM((NQ, N_DEV * ROWS, QW), bf16),
            pltpu.SemaphoreType.DMA((7 + NQ,)),
            pltpu.SemaphoreType.DMA((n_remote,)),
            pltpu.SemaphoreType.DMA((n_remote,)),
        ],
        compiler_params=pltpu.CompilerParams(collective_id=0),
    )(x, expert_W, shared_W, router_W.T,
      route_idx.astype(jnp.int32).reshape(N_DEV, ROWS))
```

```python
import jax
import jax.numpy as jnp
from jax import lax
from jax.experimental import pallas as pl
from jax.experimental.pallas import tpu as pltpu

N_DEV = 4
N_TOK = 512
D = 256
H = 512
N_EXP = 8
E_LOC = N_EXP // N_DEV
ROWS = N_TOK // N_DEV
N_REM = N_DEV - 1

NQ = 4
QW = H // NQ
CH = 16
NCH = ROWS // CH
CAP_FAST = 48
DEFER = NQ

def pallas_dist_moe_shared_ep_outshard_n512_d256_e2_h512_kernel(
    x: jax.Array,
    router_W: jax.Array,
    route_idx: jax.Array,
    expert_W: jax.Array,
    shared_W: jax.Array,
):
    f32, bf16, i32 = jnp.float32, jnp.bfloat16, jnp.int32

    def body(x_hbm, ew_hbm, sw_hbm, rwt_hbm, ridx_hbm, out_ref,
             ridx_v, rwt_v, xs_v, ew_v, sw_v, send_buf, recv_buf,
             ld_sems, send_sems, recv_sems):
        my = lax.axis_index("i")
        odd = my & 1
        peer = [lax.rem(my + 2, N_DEV),
                lax.rem(my + 1 + 2 * odd, N_DEV),
                lax.rem(my + 3 - 2 * odd, N_DEV),
                my]

        cp_ridx = pltpu.make_async_copy(ridx_hbm, ridx_v, ld_sems.at[0])
        cp_rwt = pltpu.make_async_copy(rwt_hbm, rwt_v, ld_sems.at[1])
        cp_ridx.start()
        cp_rwt.start()
        cp_x = []
        for s in range(N_DEV):
            start = pl.multiple_of(peer[s] * ROWS, ROWS)
            cp_x.append(pltpu.make_async_copy(
                x_hbm.at[pl.ds(start, ROWS)],
                xs_v.at[pl.ds(s * ROWS, ROWS)], ld_sems.at[2 + s]))
        cp_w = [pltpu.make_async_copy(ew_hbm.at[:, :, pl.ds(q * QW, QW)],
                                      ew_v.at[q], ld_sems.at[6 + q])
                for q in range(NQ)]
        cp_sw = pltpu.make_async_copy(sw_hbm, sw_v, ld_sems.at[6 + NQ])
        for s in range(N_REM):
            cp_x[s].start()
        for q in range(NQ):
            cp_w[q].start()
        cp_x[N_REM].start()
        cp_sw.start()

        recv_buf[...] = jnp.zeros(recv_buf.shape, bf16)
        bsem = pltpu.get_barrier_semaphore()
        for k in range(1, N_DEV):
            pl.semaphore_signal(bsem, inc=1,
                                device_id=(lax.rem(my + k, N_DEV),),
                                device_id_type=pl.DeviceIdType.MESH)

        cp_ridx.wait()
        r4 = ridx_v[...]
        sub4 = lax.broadcasted_iota(i32, (N_DEV, ROWS), 0)
        rows = [jnp.sum(jnp.where(sub4 == peer[s], r4, 0),
                        axis=0, keepdims=True) for s in range(N_DEV)]
        rs8 = jnp.concatenate(rows + [jnp.full((4, ROWS), -1, i32)], axis=0)
        owner8 = lax.shift_right_arithmetic(rs8, 1)
        tri = (lax.broadcasted_iota(i32, (ROWS, ROWS), 0)
               < lax.broadcasted_iota(i32, (ROWS, ROWS), 1)).astype(bf16)
        rank8 = jnp.zeros((8, ROWS), f32)
        for o in range(N_DEV):
            mo = owner8 == o
            pre = jnp.dot(mo.astype(bf16), tri, preferred_element_type=f32)
            rank8 = rank8 + jnp.where(mo, pre, 0.0)
        rank8 = rank8.astype(i32)

        mine8 = owner8 == my
        key8 = jnp.where(mine8, rank8, -1)
        n_send, n_recv = [], []
        for s in range(N_DEV):
            cnt = jnp.sum(mine8[s:s + 1, :].astype(i32))
            n_send.append((cnt + (CH - 1)) // CH)
        own_row = owner8[N_REM:N_REM + 1, :]
        slot_of = jnp.full_like(own_row, N_REM)
        for s in range(N_REM):
            slot_of = jnp.where(own_row == peer[s], s, slot_of)
        for s in range(N_REM):
            cnt = jnp.sum((slot_of == s).astype(i32))
            n_recv.append((cnt + (CH - 1)) // CH)
        pos_row = slot_of * ROWS + rank8[N_REM:N_REM + 1, :]

        cp_rwt.wait()
        rw = rwt_v[...]
        rw_hi = rw.astype(bf16)
        rw_lo = (rw - rw_hi.astype(f32)).astype(bf16)
        rw_cat = jnp.concatenate(
            [jnp.concatenate([rw_hi, rw_hi], axis=1),
             jnp.concatenate([rw_lo, jnp.zeros_like(rw_lo)], axis=1)],
            axis=0)
        nt = (((1,), (1,)), ((), ()))

        def split(xf):
            hi = xf.astype(bf16)
            lo = (xf - hi.astype(f32)).astype(bf16)
            return jnp.concatenate([hi, lo], axis=1)

        def probs_t(x_hl):
            a = lax.dot_general(rw_cat, x_hl, nt, preferred_element_type=f32)
            sc = a[0:N_EXP] + a[N_EXP:2 * N_EXP]
            mx = jnp.max(sc, axis=0, keepdims=True)
            ex = jnp.exp(sc - mx)
            return ex / jnp.sum(ex, axis=0, keepdims=True)

        def local_gates(gsel):
            sub = lax.broadcasted_iota(i32, gsel.shape, 0)
            return [jnp.sum(jnp.where(sub == my * E_LOC + e, gsel, 0.0),
                            axis=0, keepdims=True) for e in range(E_LOC)]

        def rdma(s, q, n, stride):
            idx = q * N_REM + s
            return pltpu.make_async_remote_copy(
                src_ref=send_buf.at[q, pl.ds(s * stride, n * CH), :],
                dst_ref=recv_buf.at[q, pl.ds(s * ROWS, n * CH), :],
                send_sem=send_sems.at[idx],
                recv_sem=recv_sems.at[idx],
                device_id=(peer[s],),
                device_id_type=pl.DeviceIdType.MESH)

        def by_size(n_dyn, n_max, fn, lo=0):
            if lo == n_max:
                if lo > 0:
                    fn(lo)
                return
            mid = (lo + n_max) // 2
            lax.cond(n_dyn <= mid,
                     lambda: by_size(n_dyn, mid, fn, lo),
                     lambda: by_size(n_dyn, n_max, fn, mid + 1))

        def send_phase(cap):
            m = N_REM * cap
            sub_c = lax.broadcasted_iota(i32, (cap, ROWS), 0)
            sub_e = lax.broadcasted_iota(i32, (N_EXP, ROWS), 0)
            ps = [(key8[s:s + 1, :] == sub_c).astype(bf16)
                  for s in range(N_DEV)]
            sels = [lax.dot_general(
                (sub_e == rs8[s:s + 1, :]).astype(bf16), ps[s], nt,
                preferred_element_type=f32) for s in range(N_DEV)]

            def compact(slots):
                xcs = [jnp.dot(ps[s], split(xs_v[s * ROWS:(s + 1) * ROWS, :]),
                               preferred_element_type=f32).astype(bf16)
                       for s in slots]
                xh = jnp.concatenate([xc[:, 0:D] for xc in xcs], axis=0)
                gts = []
                for s, xc in zip(slots, xcs):
                    g0, g1 = local_gates(probs_t(xc) * sels[s])
                    gts.append(jnp.concatenate(
                        [g0, g1, jnp.zeros((8 - E_LOC, cap), f32)], axis=0).T)
                gc0 = jnp.concatenate([g[:, 0:1] for g in gts], axis=0)
                gc1 = jnp.concatenate([g[:, 1:2] for g in gts], axis=0)
                return xh, gc0, gc1

            def experts(q, xh, gc0, gc1):
                wq = jnp.concatenate([ew_v[q, 0], ew_v[q, 1]],
                                     axis=1).astype(bf16)
                yy = jnp.dot(xh, wq, preferred_element_type=f32)
                return (gc0 * yy[:, 0:QW]
                        + gc1 * yy[:, QW:2 * QW]).astype(bf16)

            for s in range(N_REM):
                cp_x[s].wait()
            rem = compact(range(N_REM))
            for q in range(NQ):
                cp_w[q].wait()
                send_buf[q, 0:m, :] = experts(q, *rem)
                if q == 0:
                    pl.semaphore_wait(bsem, N_REM)
                for s, qq in ((0, q), (1, q), (2, q - DEFER)):
                    if qq >= 0:
                        by_size(n_send[s], cap // CH,
                                lambda n, s=s, qq=qq:
                                rdma(s, qq, n, cap).start())
            for qq in range(max(NQ - DEFER, 0), NQ):
                by_size(n_send[2], cap // CH,
                        lambda n, qq=qq: rdma(2, qq, n, cap).start())

            cp_x[N_REM].wait()
            own = compact([N_REM])
            for q in range(NQ):
                recv_buf[q, N_REM * ROWS:N_REM * ROWS + cap, :] = experts(q, *own)

        n_max = jnp.maximum(jnp.maximum(n_send[0], n_send[1]),
                            jnp.maximum(n_send[2], n_send[3]))
        lax.cond(n_max <= CAP_FAST // CH,
                 lambda: send_phase(CAP_FAST),
                 lambda: send_phase(ROWS))

        posc = jnp.concatenate(
            [pos_row.astype(f32), jnp.zeros((7, ROWS), f32)], axis=0).T
        lane = lax.broadcasted_iota(i32, (ROWS, N_DEV * ROWS), 1)
        qcat = (posc[:, 0:1].astype(i32) == lane).astype(bf16)
        cp_sw.wait()
        out_ref[...] = jnp.dot(
            xs_v[N_REM * ROWS:N_DEV * ROWS, :].astype(bf16),
            sw_v[...].astype(bf16), preferred_element_type=f32)

        for s in range(N_REM):
            def waits(n, s=s):
                for q in range(NQ):
                    rdma(s, q, n, ROWS).wait_send()
            by_size(n_send[s], NCH, waits)

        def scatter_add(q):
            out_ref[:, q * QW:(q + 1) * QW] += jnp.dot(
                qcat, recv_buf[q], preferred_element_type=f32)

        for s in range(N_REM):
            def waits(n, s=s):
                for q in range(NQ - 1):
                    rdma(s, q, n, ROWS).wait_recv()
            by_size(n_recv[s], NCH, waits)
        for q in range(NQ - 1):
            scatter_add(q)
        for s in range(N_REM):
            by_size(n_recv[s], NCH,
                    lambda n, s=s: rdma(s, NQ - 1, n, ROWS).wait_recv())
        scatter_add(NQ - 1)

    n_remote = NQ * N_REM
    return pl.pallas_call(
        body,
        out_shape=jax.ShapeDtypeStruct((ROWS, H), f32),
        in_specs=[pl.BlockSpec(memory_space=pltpu.HBM)] * 5,
        out_specs=pl.BlockSpec(memory_space=pltpu.VMEM),
        scratch_shapes=[
            pltpu.VMEM((N_DEV, ROWS), i32),
            pltpu.VMEM((N_EXP, D), f32),
            pltpu.VMEM((N_TOK, D), f32),
            pltpu.VMEM((NQ, E_LOC, D, QW), f32),
            pltpu.VMEM((D, H), f32),
            pltpu.VMEM((NQ, N_REM * ROWS, QW), bf16),
            pltpu.VMEM((NQ, N_DEV * ROWS, QW), bf16),
            pltpu.SemaphoreType.DMA((7 + NQ,)),
            pltpu.SemaphoreType.DMA((n_remote,)),
            pltpu.SemaphoreType.DMA((n_remote,)),
        ],
        compiler_params=pltpu.CompilerParams(collective_id=0),
    )(x, expert_W, shared_W, router_W.T,
      route_idx.astype(jnp.int32).reshape(N_DEV, ROWS))
```
